```python
import numpy as np

kernel_name = "dist_max_ax1_xy_m4096_n1024"

def setup_inputs():
    return {"x": np.random.randn(8192, 2048).astype(np.float32)}

def reference(x: np.ndarray) -> np.ndarray:
    return np.max(x, axis=1, keepdims=True)
```

```python
import jax, jax.numpy as jnp
from jax import lax
from jax.experimental import pallas as pl
from jax.experimental.pallas import tpu as pltpu

MESH = pl.DeviceIdType.MESH

def colmax(xbuf, r0, nr, N):
    t = [xbuf[pl.ds(r0, nr), c * 128:(c + 1) * 128] for c in range(N // 128)]
    while len(t) > 1:
        t = [jnp.maximum(t[i], t[i + 1]) for i in range(0, len(t), 2)]
    return t[0]

def make(tail=(96, 32), bulk=128, dbc=True, dsc=True, flags=None, name="kern"):
    assert sum(tail) == 128
    def fn(x):
        M, N = x.shape
        L = 128
        NB = M // L
        Q = M // 4
        QB = NB // 4
        chunks = [(r, bulk) for r in range(0, 3 * Q, bulk)] + [(r, L) for r in range(3 * Q, M - L, L)]
        r = M - L
        for t in tail:
            chunks.append((r, t)); r += t
        nbulk = 3 * Q // bulk
        def body(x_hbm, o_ref, xbuf, part, recv, in_sems, send_sems, recv_sems):
            def copy(i, my=None):
                r0, nr = chunks[i]
                q = r0 // Q
                if q < 2 or my is None: src = r0
                elif q == 2: src = pl.multiple_of(r0 + (1 - my) * Q, 8)
                else: src = pl.multiple_of(r0 - (1 - my) * Q, 8)
                return pltpu.make_async_copy(x_hbm.at[pl.ds(src, nr)], xbuf.at[pl.ds(r0, nr)], in_sems.at[i])
            n_common = 2 * Q // bulk
            for i in range(n_common):
                copy(i).start()
            mx = lax.axis_index("x"); my = lax.axis_index("y")
            peer = (mx, 1 - my)
            for i in range(n_common, len(chunks)):
                copy(i, my).start()
            bar = pltpu.get_barrier_semaphore()
            pl.semaphore_signal(bar, 1, device_id=peer, device_id_type=MESH)

            def block(b):
                r0 = b * L if isinstance(b, int) else pl.multiple_of(b * L, L)
                return jnp.max(colmax(xbuf, r0, L, N).T, axis=0, keepdims=True)

            def bulk_step(i, _):
                r0 = pl.multiple_of(i * bulk, bulk)
                pltpu.make_async_copy(x_hbm.at[pl.ds(r0, bulk)], xbuf.at[pl.ds(r0, bulk)], in_sems.at[i]).wait()
                for j in range(bulk // L):
                    b = i * (bulk // L) + j
                    part[pl.ds(b, 1), :] = block(b)
            lax.fori_loop(0, nbulk, bulk_step, None)

            pl.semaphore_wait(bar, 1)
            xch = pltpu.make_async_remote_copy(part.at[pl.ds(0, 3 * QB)], recv, send_sems.at[0], recv_sems.at[0], device_id=peer, device_id_type=MESH)
            xch.start()

            def last_step(j, _):
                r0 = pl.multiple_of(3 * Q + j * L, L)
                pltpu.make_async_copy(x_hbm.at[pl.ds(r0, L)], xbuf.at[pl.ds(r0, L)], in_sems.at[nbulk + j]).wait()
                part[pl.ds(3 * QB + j, 1), :] = block(3 * QB + j)
            lax.fori_loop(0, QB - 1, last_step, None)

            xch.wait_recv()
            o0 = pl.multiple_of((2 + my) * QB, QB)
            o_ref[pl.ds(o0, QB - 1), :] = jnp.maximum(part[pl.ds(3 * QB, QB - 1), :], recv[pl.ds(2 * QB, QB - 1), :])
            fin0 = pltpu.make_async_remote_copy(o_ref.at[pl.ds(o0, QB - 1)], o_ref.at[pl.ds(o0, QB - 1)], send_sems.at[1], recv_sems.at[1], device_id=peer, device_id_type=MESH)
            fin0.start()
            o_ref[pl.ds(0, 2 * QB), :] = jnp.maximum(part[pl.ds(0, 2 * QB), :], recv[pl.ds(0, 2 * QB), :])
            xch.wait_send()

            lane = lax.broadcasted_iota(jnp.int32, (8, L), 1)
            sub = lax.broadcasted_iota(jnp.int32, (8, L), 0)
            d = lane - sub
            acc = jnp.broadcast_to(recv[pl.ds(3 * QB - 1, 1), :], (8, L))
            i = nbulk + QB - 1
            for t in tail:
                r0, nr = chunks[i]
                copy(i).wait()
                for g in range(r0, r0 + nr, 8):
                    m = jnp.max(colmax(xbuf, g, 8, N), axis=1, keepdims=True)
                    acc = jnp.where(d == (g - (M - L)), jnp.maximum(acc, m), acc)
                i += 1
            o_ref[pl.ds(o0 + QB - 1, 1), :] = jnp.max(acc, axis=0, keepdims=True)
            fin1 = pltpu.make_async_remote_copy(o_ref.at[pl.ds(o0 + QB - 1, 1)], o_ref.at[pl.ds(o0 + QB - 1, 1)], send_sems.at[2], recv_sems.at[2], device_id=peer, device_id_type=MESH)
            fin1.start()
            fin0.wait_send()
            fin1.wait_send()
            fin0.wait_recv()
            fin1.wait_recv()

        out = pl.pallas_call(
            body,
            out_shape=jax.ShapeDtypeStruct((NB, L), x.dtype),
            in_specs=[pl.BlockSpec(memory_space=pl.ANY)],
            out_specs=pl.BlockSpec(memory_space=pltpu.VMEM),
            scratch_shapes=[pltpu.VMEM((M, N), x.dtype), pltpu.VMEM((NB, L), x.dtype), pltpu.VMEM((3 * QB, L), x.dtype),
                            pltpu.SemaphoreType.DMA((len(chunks),)), pltpu.SemaphoreType.DMA((3,)), pltpu.SemaphoreType.DMA((3,))],
            compiler_params=pltpu.CompilerParams(collective_id=0, vmem_limit_bytes=32 * 2**20, disable_bounds_checks=dbc, disable_semaphore_checks=dsc, flags=flags),
            name=name,
        )(x)
        return out.reshape(M, 1)
    return fn


def pallas_dist_max_ax1_xy_m4096_n1024_kernel(x):
    return make()(x)
```

```python
import jax
import jax.numpy as jnp
from jax import lax
from jax.experimental import pallas as pl
from jax.experimental.pallas import tpu as pltpu

BLOCK = 128
SUBLANES = 8

ROWS_TO_Y = 216
ROWS_TO_X = 184
EARLY_CHUNKS = (16, 4, 2, 1)
LATE_CHUNKS = (1, 1, 1)
LAST_BLOCK_CHUNKS = (96, 32)


def _fold_columns(ref, row, n_rows):
    tiles = [
        ref[pl.ds(row, n_rows), c : c + BLOCK] for c in range(0, ref.shape[1], BLOCK)
    ]
    while len(tiles) > 1:
        tiles = [jnp.maximum(a, b) for a, b in zip(tiles[::2], tiles[1::2])]
    return tiles[0]


def _row_maxima(ref, row, n_rows=BLOCK, first_lane=0):
    folded = _fold_columns(ref, row, n_rows)

    def filler(n):
        return [jnp.full((n, BLOCK), -jnp.inf, folded.dtype)] if n else []

    square = jnp.concatenate(
        filler(first_lane) + [folded] + filler(BLOCK - first_lane - n_rows), axis=0
    )
    return jnp.max(square.T, axis=0, keepdims=True)


def _row_max_kernel(
    x_hbm, out_ref,
    rows, rows_from_y, rows_from_x, partial, peer_partial, for_x, from_x,
    chunk_sems, load_sems, send_sems, recv_sems,
):
    n_blocks = out_ref.shape[0]
    x_block = n_blocks - 6
    y_block = n_blocks - 4
    kept_x = 2 * BLOCK - ROWS_TO_X
    kept_y = 2 * BLOCK - ROWS_TO_Y
    their_slot = y_block * BLOCK
    my_slot = (y_block + 2) * BLOCK

    def load(src_row, dst_row, n_rows, sem):
        copy = pltpu.make_async_copy(
            x_hbm.at[pl.ds(src_row, n_rows)], rows.at[pl.ds(dst_row, n_rows)], sem
        )
        copy.start()
        return copy

    def remote(src, dst, i, device):
        return pltpu.make_async_remote_copy(
            src, dst, send_sems.at[i], recv_sems.at[i],
            device_id=device, device_id_type=pl.DeviceIdType.MESH,
        )

    load_x = load(x_block * BLOCK, x_block * BLOCK, kept_x, load_sems.at[0])

    my_x, my_y = lax.axis_index("x"), lax.axis_index("y")
    y_peer, x_peer = (my_x, 1 - my_y), (1 - my_x, my_y)
    my_block = y_block + 2 * my_y
    their_block = y_block + 2 * (1 - my_y)

    def row_of(block, offset=0):
        return pl.multiple_of(block * BLOCK + offset, SUBLANES)

    barrier = pltpu.get_barrier_semaphore()
    for peer in (y_peer, x_peer):
        pl.semaphore_signal(
            barrier, 1, device_id=peer, device_id_type=pl.DeviceIdType.MESH
        )

    load_theirs = load(row_of(their_block), their_slot, kept_y, load_sems.at[1])
    chunks, block = [], 0
    for i, n in enumerate(EARLY_CHUNKS + LATE_CHUNKS):
        copy = load(block * BLOCK, block * BLOCK, n * BLOCK, chunk_sems.at[i])
        chunks.append((block, copy))
        block += n
    assert block == x_block
    load_mine = load(row_of(my_block), my_slot, BLOCK, load_sems.at[2])
    last_chunks, row = [], 0
    for i, n in enumerate(LAST_BLOCK_CHUNKS):
        copy = load(
            row_of(my_block + 1, row), my_slot + BLOCK + row, n, load_sems.at[3 + i]
        )
        last_chunks.append((row, n, copy))
        row += n
    assert row == BLOCK

    pl.semaphore_wait(barrier, 2)
    raw_y = remote(
        x_hbm.at[pl.ds(row_of(their_block, kept_y), ROWS_TO_Y)], rows_from_y, 0, y_peer
    )
    raw_x = remote(
        x_hbm.at[pl.ds(x_block * BLOCK + kept_x, ROWS_TO_X)], rows_from_x, 1, x_peer
    )
    raw_y.start()
    raw_x.start()
    reply_x = remote(for_x, from_x, 2, x_peer)

    partial[...] = jnp.full(partial.shape, -jnp.inf, partial.dtype)
    load_x.wait()
    partial[pl.ds(x_block, 1), :] = _row_maxima(rows, x_block * BLOCK, kept_x)
    load_theirs.wait()
    partial[pl.ds(their_block, 1), :] = _row_maxima(rows, their_slot, kept_y)

    def plain_block(b, carry):
        for first, copy in chunks:
            pl.when(b == first)(copy.wait)
        partial[pl.ds(b, 1), :] = _row_maxima(rows, row_of(b))

        @pl.when(b == sum(EARLY_CHUNKS) - 1)
        def _():
            raw_x.wait_recv()
            for_x[0:1, :] = _row_maxima(rows_from_x, 0, BLOCK - kept_x, kept_x)
            for_x[1:2, :] = _row_maxima(rows_from_x, BLOCK - kept_x)
            reply_x.start()

        return carry

    lax.fori_loop(0, x_block, plain_block, None)

    raw_y.wait_recv()
    peer_first = _row_maxima(rows_from_y, 0, BLOCK - kept_y, kept_y)
    peer_last = _row_maxima(rows_from_y, BLOCK - kept_y)
    load_mine.wait()
    partial[pl.ds(my_block, 1), :] = jnp.maximum(peer_first, _row_maxima(rows, my_slot))
    reply_x.wait_recv()
    x_rows = pl.ds(x_block, 2)
    partial[x_rows, :] = jnp.maximum(partial[x_rows, :], from_x[...])
    exchange = remote(partial, peer_partial, 3, y_peer)
    exchange.start()

    tile = (SUBLANES, BLOCK)
    lane = lax.broadcasted_iota(jnp.int32, tile, 1)
    diagonal = lane - lax.broadcasted_iota(jnp.int32, tile, 0)
    result = jnp.broadcast_to(peer_last, tile)
    for first, n, copy in last_chunks:
        copy.wait()
        placed = jnp.full(tile, -jnp.inf, result.dtype)
        for r in range(first, first + n, SUBLANES):
            folded = _fold_columns(rows, my_slot + BLOCK + r, SUBLANES)
            maxima = jnp.max(folded, axis=1, keepdims=True)
            placed = jnp.where(diagonal == r, maxima, placed)
        result = jnp.maximum(result, placed)
    my_last = pl.ds(my_block + 1, 1)
    out_ref[my_last, :] = jnp.max(result, axis=0, keepdims=True)
    final = remote(out_ref.at[my_last], out_ref.at[my_last], 4, y_peer)
    final.start()

    for copy in (raw_y, raw_x, reply_x, exchange, final):
        copy.wait_send()
    exchange.wait_recv()
    for done in (pl.ds(0, y_block + 1), pl.ds(y_block + 2, 1)):
        out_ref[done, :] = jnp.maximum(partial[done, :], peer_partial[done, :])
    their_last = out_ref.at[pl.ds(their_block + 1, 1)]
    remote(their_last, their_last, 4, y_peer).wait_recv()


def pallas_dist_max_ax1_xy_m4096_n1024_kernel(x: jax.Array):
    m, n = x.shape
    results = (m // BLOCK, BLOCK)

    def body(*refs):
        dma = pltpu.SemaphoreType.DMA
        pl.run_scoped(
            lambda *sems: _row_max_kernel(*refs, *sems),
            dma((len(EARLY_CHUNKS + LATE_CHUNKS),)),
            dma((3 + len(LAST_BLOCK_CHUNKS),)),
            dma((5,)),
            dma((5,)),
        )

    out = pl.pallas_call(
        body,
        out_shape=jax.ShapeDtypeStruct(results, x.dtype),
        in_specs=[pl.BlockSpec(memory_space=pl.ANY)],
        out_specs=pl.BlockSpec(memory_space=pltpu.VMEM),
        scratch_shapes=[
            pltpu.VMEM((m, n), x.dtype),
            pltpu.VMEM((ROWS_TO_Y, n), x.dtype),
            pltpu.VMEM((ROWS_TO_X, n), x.dtype),
            pltpu.VMEM(results, x.dtype),
            pltpu.VMEM(results, x.dtype),
            pltpu.VMEM((2, BLOCK), x.dtype),
            pltpu.VMEM((2, BLOCK), x.dtype),
        ],
        compiler_params=pltpu.CompilerParams(
            collective_id=0, vmem_limit_bytes=32 * 1024 * 1024
        ),
    )(x)
    return out.reshape(m, 1)
```
